```python
import numpy as np

kernel_name = "dist_mean_ax1_xy_m4096_n1024"

def setup_inputs():
    return {"x": np.random.randn(8192, 2048).astype(np.float32)}

def reference(x: np.ndarray) -> np.ndarray:
    return np.mean(x, axis=1, keepdims=True)
```

```python
import jax
import jax.numpy as jnp
from jax import lax
from jax.experimental import pallas as pl
from jax.experimental.pallas import tpu as pltpu

M, N = 4096, 1024
H = M // 2
BLK = 128
RAW = 192
RAW_FULL = RAW // BLK * BLK
HEAD = (H - RAW,)
BODY = (1280, 512, 128)
TAIL = (96, 32)
SCALE = 1.0 / (2 * N)
MESH = pl.DeviceIdType.MESH


def _row_sums(ref, r0, nrows=BLK, lane0=0):
    cols = [ref[pl.ds(r0, nrows), j * 128:(j + 1) * 128] for j in range(N // 128)]
    while len(cols) > 1:
        cols = [cols[k] + cols[k + 1] for k in range(0, len(cols), 2)]
    folded = cols[0]
    lanes = lax.broadcasted_iota(jnp.int32, (8, 128), 1)
    sublanes = lax.broadcasted_iota(jnp.int32, (8, 128), 0)
    groups = [None] * (BLK // 8)
    for g in range(nrows // 8):
        groups[lane0 // 8 + g] = jnp.sum(
            folded[8 * g:8 * g + 8], axis=1, keepdims=True)
    bit = 3
    while len(groups) > 1:
        upper = ((lanes >> bit) & 1) == 1
        merged = []
        for lo, hi in zip(groups[0::2], groups[1::2]):
            if lo is None and hi is None:
                merged.append(None)
            else:
                merged.append(jnp.where(upper,
                                        0.0 if hi is None else hi,
                                        0.0 if lo is None else lo))
        groups = merged
        bit += 1
    diag = jnp.where((lanes & 7) == sublanes, groups[0], 0.0)
    return jnp.sum(diag, axis=0, keepdims=True)


def pallas_dist_mean_ax1_xy_m4096_n1024_kernel(x):
    chunks = HEAD + BODY + TAIL
    n_head, n_body, n = len(HEAD), len(BODY), len(HEAD + BODY + TAIL)
    starts = [RAW + sum(chunks[:i]) for i in range(n)]
    early = sum(BODY)

    def body(x_hbm, out_ref, xbuf, rawbuf, part, recv, fin,
             in_sems, send_sem, raw_sem, part_sem, fin_sem):
        my = lax.axis_index("y")
        peer = (lax.axis_index("x"), 1 - my)
        own = pl.multiple_of(my * H, H)
        other = pl.multiple_of((1 - my) * H, H)

        def load(i):
            src = other + starts[i] if i < n_head else own + (starts[i] - H)
            return pltpu.make_async_copy(
                x_hbm.at[pl.ds(src, chunks[i]), :],
                xbuf.at[pl.ds(starts[i], chunks[i]), :],
                in_sems.at[i])

        def remote(src, dst, recv_sem):
            return pltpu.make_async_remote_copy(
                src, dst, send_sem, recv_sem, device_id=peer, device_id_type=MESH)

        def reduce_chunk(i):
            r, end = starts[i], starts[i] + chunks[i]
            if r % BLK:
                k = BLK - r % BLK
                part[:, pl.ds(r - r % BLK, BLK)] = _row_sums(xbuf, r, k, r % BLK)
                r += k
            nb = (end - r) // BLK
            if nb == 1:
                part[:, pl.ds(r, BLK)] = _row_sums(xbuf, r)
            else:
                def step(b, carry):
                    r0 = pl.multiple_of(r + b * BLK, BLK)
                    part[:, pl.ds(r0, BLK)] = _row_sums(xbuf, r0)
                    return carry
                lax.fori_loop(0, nb, step, 0)

        for i in range(n):
            load(i).start()

        barrier = pltpu.get_barrier_semaphore()
        pl.semaphore_signal(barrier, inc=1, device_id=peer, device_id_type=MESH)
        pl.semaphore_wait(barrier, 1)

        send_raw = remote(x_hbm.at[pl.ds(other, RAW), :], rawbuf, raw_sem)
        send_raw.start()

        for i in range(n_head):
            load(i).wait()
            reduce_chunk(i)
        send_part = remote(part.at[:, pl.ds(RAW_FULL, H - RAW_FULL)],
                           recv.at[:, pl.ds(RAW_FULL, H - RAW_FULL)], part_sem)
        send_part.start()

        for i in range(n_head, n_head + n_body):
            load(i).wait()
            reduce_chunk(i)
            if i == n_head + 1:
                send_raw.wait_recv()
                for r in range(0, RAW_FULL, BLK):
                    recv[:, pl.ds(r, BLK)] = _row_sums(rawbuf, r)
                if RAW > RAW_FULL:
                    sl = pl.ds(H + RAW_FULL, BLK)
                    part[:, sl] = part[:, sl] + _row_sums(
                        rawbuf, RAW_FULL, RAW - RAW_FULL, 0)

        def send_final(off, size):
            return remote(fin.at[:, pl.ds(off, size)],
                          out_ref.at[:, pl.ds(own + off, size)], fin_sem)

        send_part.wait_recv()
        means = (part[:, pl.ds(H, early)] + recv[:, pl.ds(0, early)]) * SCALE
        fin[:, pl.ds(0, early)] = means
        send_early = send_final(0, early)
        send_early.start()
        out_ref[:, pl.ds(own, early)] = means

        acc = recv[:, pl.ds(early, BLK)]
        for i in range(n_head + n_body, n):
            load(i).wait()
            acc = acc + _row_sums(xbuf, starts[i], chunks[i], starts[i] % BLK)
        means = acc * SCALE
        fin[:, pl.ds(early, BLK)] = means
        send_late = send_final(early, BLK)
        send_late.start()
        out_ref[:, pl.ds(pl.multiple_of(own + early, BLK), BLK)] = means

        send_raw.wait_send()
        send_part.wait_send()
        send_early.wait_send()
        send_late.wait_send()
        pltpu.make_async_copy(fin, fin, fin_sem).wait()

    out = pl.pallas_call(
        body,
        out_shape=jax.ShapeDtypeStruct((1, M), jnp.float32),
        in_specs=[pl.BlockSpec(memory_space=pl.ANY)],
        out_specs=pl.BlockSpec(memory_space=pltpu.VMEM),
        scratch_shapes=[
            pltpu.VMEM((M, N), jnp.float32),
            pltpu.VMEM((RAW, N), jnp.float32),
            pltpu.VMEM((1, M), jnp.float32),
            pltpu.VMEM((1, H), jnp.float32),
            pltpu.VMEM((1, H), jnp.float32),
            pltpu.SemaphoreType.DMA((n,)),
            pltpu.SemaphoreType.DMA,
            pltpu.SemaphoreType.DMA,
            pltpu.SemaphoreType.DMA,
            pltpu.SemaphoreType.DMA,
        ],
        compiler_params=pltpu.CompilerParams(
            collective_id=0,
            vmem_limit_bytes=64 * 1024 * 1024,
            disable_semaphore_checks=True,
            disable_bounds_checks=True,
        ),
    )(x)
    return out.reshape(M, 1)
```

```python
import jax
import jax.numpy as jnp
from jax import lax
from jax.experimental import pallas as pl
from jax.experimental.pallas import tpu as pltpu

M, N = 4096, 1024
H = M // 2
BLK = 128
RAW = 192
RAW_FULL = RAW // BLK * BLK
HEAD = (H - RAW,)
BODY = (1280, 512, 128)
TAIL = (96, 32)
SCALE = 1.0 / (2 * N)
MESH = pl.DeviceIdType.MESH


def _row_sums(ref, r0, nrows=BLK, lane0=0):
    cols = [ref[pl.ds(r0, nrows), j * 128:(j + 1) * 128] for j in range(N // 128)]
    while len(cols) > 1:
        cols = [cols[k] + cols[k + 1] for k in range(0, len(cols), 2)]
    folded = cols[0]
    lanes = lax.broadcasted_iota(jnp.int32, (8, 128), 1)
    sublanes = lax.broadcasted_iota(jnp.int32, (8, 128), 0)
    groups = [None] * (BLK // 8)
    for g in range(nrows // 8):
        groups[lane0 // 8 + g] = jnp.sum(
            folded[8 * g:8 * g + 8], axis=1, keepdims=True)
    bit = 3
    while len(groups) > 1:
        upper = ((lanes >> bit) & 1) == 1
        groups = [hi if lo is None else lo if hi is None
                  else jnp.where(upper, hi, lo)
                  for lo, hi in zip(groups[0::2], groups[1::2])]
        bit += 1
    keep = (lanes & 7) == sublanes
    if nrows < BLK:
        keep = keep & (lanes >= lane0) & (lanes < lane0 + nrows)
    diag = jnp.where(keep, groups[0], 0.0)
    return jnp.sum(diag, axis=0, keepdims=True)


def pallas_dist_mean_ax1_xy_m4096_n1024_kernel(x):
    chunks = HEAD + BODY + TAIL
    n_head, n_body, n = len(HEAD), len(BODY), len(HEAD + BODY + TAIL)
    starts = [RAW + sum(chunks[:i]) for i in range(n)]
    early = sum(BODY)

    def body(x_hbm, out_ref, xbuf, rawbuf, part, recv, fin,
             in_sems, send_sem, raw_sem, part_sem, fin_sem):
        my = lax.axis_index("y")
        peer = (lax.axis_index("x"), 1 - my)
        own = pl.multiple_of(my * H, H)
        other = pl.multiple_of((1 - my) * H, H)

        def load(i):
            src = other + starts[i] if i < n_head else own + (starts[i] - H)
            return pltpu.make_async_copy(
                x_hbm.at[pl.ds(src, chunks[i]), :],
                xbuf.at[pl.ds(starts[i], chunks[i]), :],
                in_sems.at[i])

        def remote(src, dst, recv_sem):
            return pltpu.make_async_remote_copy(
                src, dst, send_sem, recv_sem, device_id=peer, device_id_type=MESH)

        def reduce_chunk(i):
            r, end = starts[i], starts[i] + chunks[i]
            if r % BLK:
                k = BLK - r % BLK
                part[:, pl.ds(r - r % BLK, BLK)] = _row_sums(xbuf, r, k, r % BLK)
                r += k
            nb = (end - r) // BLK
            if nb == 1:
                part[:, pl.ds(r, BLK)] = _row_sums(xbuf, r)
            else:
                def step(b, carry):
                    r0 = pl.multiple_of(r + b * BLK, BLK)
                    part[:, pl.ds(r0, BLK)] = _row_sums(xbuf, r0)
                    return carry
                lax.fori_loop(0, nb, step, 0)

        for i in range(n):
            load(i).start()

        barrier = pltpu.get_barrier_semaphore()
        pl.semaphore_signal(barrier, inc=1, device_id=peer, device_id_type=MESH)
        pl.semaphore_wait(barrier, 1)

        send_raw = remote(x_hbm.at[pl.ds(other, RAW), :], rawbuf, raw_sem)
        send_raw.start()

        for i in range(n_head):
            load(i).wait()
            reduce_chunk(i)
        send_part = remote(part.at[:, pl.ds(RAW_FULL, H - RAW_FULL)],
                           recv.at[:, pl.ds(RAW_FULL, H - RAW_FULL)], part_sem)
        send_part.start()

        for i in range(n_head, n_head + n_body):
            load(i).wait()
            reduce_chunk(i)
            if i == n_head + 1:
                send_raw.wait_recv()
                for r in range(0, RAW_FULL, BLK):
                    recv[:, pl.ds(r, BLK)] = _row_sums(rawbuf, r)
                if RAW > RAW_FULL:
                    sl = pl.ds(H + RAW_FULL, BLK)
                    part[:, sl] = part[:, sl] + _row_sums(
                        rawbuf, RAW_FULL, RAW - RAW_FULL, 0)

        def send_final(off, size):
            return remote(fin.at[:, pl.ds(off, size)],
                          out_ref.at[:, pl.ds(own + off, size)], fin_sem)

        send_part.wait_recv()
        means = (part[:, pl.ds(H, early)] + recv[:, pl.ds(0, early)]) * SCALE
        fin[:, pl.ds(0, early)] = means
        send_early = send_final(0, early)
        send_early.start()
        out_ref[:, pl.ds(own, early)] = means

        acc = recv[:, pl.ds(early, BLK)]
        for i in range(n_head + n_body, n):
            load(i).wait()
            acc = acc + _row_sums(xbuf, starts[i], chunks[i], starts[i] % BLK)
        means = acc * SCALE
        fin[:, pl.ds(early, BLK)] = means
        send_late = send_final(early, BLK)
        send_late.start()
        out_ref[:, pl.ds(pl.multiple_of(own + early, BLK), BLK)] = means

        send_raw.wait_send()
        send_part.wait_send()
        send_early.wait_send()
        send_late.wait_send()
        pltpu.make_async_copy(fin, fin, fin_sem).wait()

    out = pl.pallas_call(
        body,
        out_shape=jax.ShapeDtypeStruct((1, M), jnp.float32),
        in_specs=[pl.BlockSpec(memory_space=pl.ANY)],
        out_specs=pl.BlockSpec(memory_space=pltpu.VMEM),
        scratch_shapes=[
            pltpu.VMEM((M, N), jnp.float32),
            pltpu.VMEM((RAW, N), jnp.float32),
            pltpu.VMEM((1, M), jnp.float32),
            pltpu.VMEM((1, H), jnp.float32),
            pltpu.VMEM((1, H), jnp.float32),
            pltpu.SemaphoreType.DMA((n,)),
            pltpu.SemaphoreType.DMA,
            pltpu.SemaphoreType.DMA,
            pltpu.SemaphoreType.DMA,
            pltpu.SemaphoreType.DMA,
        ],
        compiler_params=pltpu.CompilerParams(
            collective_id=0,
            vmem_limit_bytes=64 * 1024 * 1024,
            disable_semaphore_checks=True,
            disable_bounds_checks=True,
        ),
    )(x)
    return out.reshape(M, 1)
```
